```python
import numpy as np

kernel_name = "dist_sparse_attn_causalblk_htp_bs_b2_sq256_skv256_hq4_dh64"

def setup_inputs():
    x = np.random.randn(8, 256, 512).astype(np.float32)
    Wq = np.random.randn(512, 1024).astype(np.float32) * 0.02
    K_ext = np.random.randn(8, 256, 16, 64).astype(np.float32)
    V_ext = np.random.randn(8, 256, 16, 64).astype(np.float32)
    Wo = np.random.randn(1024, 512).astype(np.float32) * 0.02
    return {"x": x, "Wq": Wq, "K_ext": K_ext, "V_ext": V_ext, "Wo": Wo}

def reference(x, Wq, K_ext, V_ext, Wo):
    B, Sq, Skv, Hq, Dh = 8, 256, 256, 16, 64
    Q = (x @ Wq).reshape(B, Sq, Hq, Dh)
    qb = (np.arange(Sq) // 64)[:, None]
    kb = (np.arange(Skv) // 64)[None, :]
    mask = kb <= qb
    scores = np.einsum('bihd,bjhd->bhij', Q, K_ext).astype(np.float32) * 0.125
    scores = np.where(mask[None, None, :, :], scores, -1e9)
    scores_max = scores.max(axis=-1, keepdims=True)
    w = np.exp(scores - scores_max)
    row_keep = mask.any(axis=1)
    w_sum = np.where(row_keep[None, None, :, None], w.sum(axis=-1, keepdims=True), 1.0)
    w = w / w_sum
    w = np.where(row_keep[None, None, :, None], w, 0.0)
    ctx = np.einsum('bhij,bjhd->bihd', w, V_ext).reshape(B, Sq, Hq * Dh)
    return ctx @ Wo
```

```python
import functools
import math

import jax
import jax.numpy as jnp
import numpy as np
from jax import lax
from jax.experimental import pallas as pl
from jax.experimental.pallas import tpu as pltpu

B = 2
S = 256
D = 512
BLK = 64
NB = S // BLK
LANES = 128
SUB = 8
SCALE = 0.125 * math.log2(math.e)
F32, BF16, I32 = jnp.float32, jnp.bfloat16, jnp.int32
MESH = pl.DeviceIdType.MESH

WO = D // 2
LOW_Q, PLANES_Q, STREAM, PLANES_O, LOW_O, END = 0, 128, 168, 184, 224, 352
CUTS = (0, 32, 64, 128, 224, D)
P_ROWS = (0, 32, 96, 192, 320)


def to_words(v):
    return pltpu.bitcast(v.astype(BF16), I32)


def to_bf16(v):
    return pltpu.bitcast(v, BF16)


def vregs(a):
    return [a[i:i + SUB] for i in range(0, a.shape[0], SUB)]


def cat(v):
    return jnp.concatenate(v, 0)


def _i32(v):
    return np.uint32(v).view(np.int32)


MAG, SIGN, BYTE, ONE = (_i32(v) for v in (0x7FFF7FFF, 0x80008000, 0x00FF00FF, 0x01000100))
RUN = 8
shl, shr = lax.shift_left, lax.shift_right_logical


def shift(x, n):
    if n == 0:
        return x
    return shl(x, np.int32(n)) if n > 0 else shr(x, np.int32(-n))


def upper_sublanes():
    return lax.broadcasted_iota(I32, (SUB, LANES), 0) >= SUB // 2


def pack_low(words):
    return [(a & BYTE) | shift(b & BYTE, 8) for a, b in zip(words[0::2], words[1::2])]


def running_max(words, acc):
    hi = functools.reduce(jnp.maximum, [a & MAG for a in words] + acc[:1])
    lo = functools.reduce(jnp.maximum, [a & 0x7FFF for a in words] + acc[1:])
    return [hi, lo]


def column_max(acc):
    hi, lo = (jnp.max(v, axis=0, keepdims=True) for v in acc)
    return (hi & _i32(0xFFFF0000)) | lo


def pack_high(words, top):
    top = jnp.broadcast_to(top, words[0].shape)
    fives, runs = [], []
    for k, a in enumerate(words):
        sign = a & SIGN if k == 0 else sign | shift(a & SIGN, -k)
        d = top - (a & MAG)
        classes = (shift(d, -8) & 0xFF, shift(d, -24))
        if k % RUN == 0:
            bits, pos = jnp.zeros_like(a), jnp.full_like(a, -1)
        if k < 15:
            far = shift((d + 0x7E007E00) & SIGN, -15)
            trit = far + shift((d + 0x7F007F00) & SIGN, -15)
            five = trit if k % 5 == 0 else five + shift(five, 1) + trit
            if k % 5 == 4:
                fives.append(five + (shift(five * 55 + 0x03FF03FF, -10) & 0x000F000F))
            for c, e in zip(classes, (far & 1, shift(far, -16))):
                pos = pos + ((c - 1) & -e)
                bits = bits | shl(e, pos & 31)
        else:
            for c in classes:
                pos = pos + c + 1
                bits = bits | shl(jnp.ones_like(a), pos & 31)
        if k % RUN == RUN - 1:
            runs += [bits, (pos + 1) & 31]
    return [sign] + fives + runs


def join_planes(a, b):
    return [a[0], b[0]] + [a[j] | shift(b[j], 8) for j in (1, 2, 3)]


def join_runs(runs):
    r = [runs[-1][0]] + [jnp.zeros_like(runs[0][0])] * 2
    for bits, n in reversed(runs[:-1]):
        r = [shl(r[0], n) | bits] + [shl(r[i], n) | shr(shift(r[i - 1], -1), 31 - n) for i in (1, 2)]
    spare = [jnp.sum(jnp.where(upper_sublanes(), 0, r[2]), axis=0, keepdims=True),
             jnp.sum(jnp.where(upper_sublanes(), r[2], 0), axis=0, keepdims=True)]
    return r[:2], spare


def unpack_high(planes, top, r):
    signs, trits = planes[:2], planes[2:]
    top = jnp.broadcast_to(top & MAG, signs[0].shape)
    out = []
    for k in range(32):
        if k % RUN == 0:
            bits, used = r[0], None
        if k % 16 < 15:
            if k % 16 % 5 == 0:
                x = shift(trits[k % 16 // 5], -8 * (k // 16))
            x = x & BYTE
            x = x + shift(x, 1)
            base = top - ((x | shift(x, -1)) & ONE)
            unary = (shift(x, -9) & 1, shift(x, -25))
        else:
            base, unary = top + ONE, (1, 1)
        extra = []
        for at, e in zip((8, 24), unary):
            n = lax.population_count(bits ^ (bits - e))
            bits = shr(bits, n)
            extra.append(shift(n, at))
        extra = extra[0] + extra[1]
        out.append(base - extra + (shift(signs[k // 16], k % 16) & SIGN))
        used = extra if used is None else used + extra
        if k % RUN == RUN - 1:
            n = (shift(used, -8) + shift(used, -24)) & 31
            r = [bits | shl(shift(r[1], 1), 31 - n),
                 shr(r[1], n) | shl(shift(r[2], 1), 31 - n),
                 shr(r[2], n)]
    return out, r


def unpack_low(high, low, top):
    top = jnp.broadcast_to(top | ONE, low[0].shape)
    out = []
    for j, packed in enumerate(low):
        for k, byte in enumerate((packed & BYTE, shift(packed, -8) & BYTE)):
            out.append(high[2 * j + k] - ((top - byte) & BYTE))
    return out


def first_half(rows):
    return lax.broadcasted_iota(I32, (rows, LANES), 1) < BLK


def scores(q, k):
    h = BLK // 2
    out = [[None] * NB for _ in range(B)]
    for qb in reversed(range(NB)):
        for b in range(B):
            block = q[(b * NB + qb) * h:(b * NB + qb + 1) * h]
            h0, h1 = jnp.where(first_half(h), block, 0), jnp.where(first_half(h), 0, block)
            rhs = to_bf16(cat([h0, h1] if qb % 2 == 0 else [h1, h0]))
            out[b][qb] = lax.dot_general(
                k[b][:(qb + 1) * BLK], rhs, (((1,), (1,)), ((), ())), preferred_element_type=F32)
    return out


def softmax(s):
    e = [jnp.exp2(v - jnp.max(v, axis=0, keepdims=True)) for v in s]
    total = [jnp.sum(v, axis=0, keepdims=True) for v in e]
    inv = [1.0 / v for v in total]
    return [to_words(v) for v in e], inv


def context(e, inv, vt, t):
    h = BLK // 2
    a, b = e[2 * t], e[2 * t + 1]
    n = a.shape[0]
    p0 = to_bf16(cat([jnp.where(first_half(n), a, b[:n]), jnp.where(first_half(h), 0, b[n:])]))
    p1 = to_bf16(cat([jnp.where(first_half(n), b[:n], a), jnp.where(first_half(h), b[n:], 0)]))
    keys = p0.shape[0]
    c0 = jnp.dot(vt[:BLK, :keys].astype(BF16), p0, preferred_element_type=F32)
    c1 = jnp.dot(vt[BLK:, :keys].astype(BF16), p1, preferred_element_type=F32)
    c0 = c0 * jnp.where(first_half(1), inv[2 * t], inv[2 * t + 1])
    c1 = c1 * jnp.where(first_half(1), inv[2 * t + 1], inv[2 * t])
    c = pltpu.bitcast(cat([c0, c1]).astype(BF16).T, I32)
    return cat([jnp.where(first_half(h), c[:h], c[h:]), jnp.where(first_half(h), c[h:], c[:h])])


def kernel_body(x_hbm, wq_hbm, k_hbm, v_hbm, wo_hbm, out_ref,
                wq32, wo32, x32, k32, v32, head32,
                w, plain, msg, top_q, top_o, parts,
                xb, qbuf, kbuf, pbuf, ctx, acc,
                load_sem, send_sem, recv_sem, ready):
    load_ids = iter(range(load_sem.shape[0]))
    copy_ids = iter(range(2, send_sem.shape[0]))

    def load(src, dst):
        copy = pltpu.make_async_copy(src, dst, load_sem.at[next(load_ids)])
        copy.start()
        return copy

    def remote(src, dst, to, sem=None):
        sem = next(copy_ids) if sem is None else sem
        return pltpu.make_async_remote_copy(
            src, dst, send_sem.at[sem], recv_sem.at[sem], device_id=(to,), device_id_type=MESH)

    def start(*groups):
        for group in groups:
            for copy in group:
                copy.start()

    def received(*groups):
        for group in groups:
            for copy in group:
                copy.wait_recv()

    def sent(*groups):
        for group in groups:
            for copy in group:
                copy.wait_send()

    def loaded(*copies):
        for copy in copies:
            copy.wait()

    pieces = tuple(zip(CUTS[:-1], CUTS[1:]))
    ld_wq = [load(wq_hbm.at[a:b], wq32.at[a:b]) for a, b in pieces]

    me = lax.axis_index("i")
    left, right, diag = (me + 3) & 3, (me + 1) & 3, me ^ 2
    odd = (me & 1) == 1

    barrier = pltpu.get_barrier_semaphore()
    head = [remote(wq_hbm.at[0:CUTS[1], LANES:], head32.at[0], right, 0),
            remote(wq_hbm.at[0:CUTS[1], :LANES], head32.at[1], left, 1)]
    packed_head = [remote(msg.at[1, 0:SUB], msg.at[3, 0:SUB], right, 0),
                   remote(msg.at[0, 0:SUB], msg.at[4, 0:SUB], left, 1)]

    @pl.when(me != 2)
    def _():
        for peer in (left, right):
            pl.semaphore_signal(barrier, 1, device_id=(peer,), device_id_type=MESH)

    @pl.when(odd)
    def _():
        pl.semaphore_wait(barrier, 1)
        pl.when(me == 3)(head[0].start)
        pl.when(me == 1)(head[1].start)

    ld_wo = [load(wo_hbm.at[h * LANES:(h + 1) * LANES], wo32.at[h]) for h in range(2)]
    ld_x = [load(x_hbm.at[b], x32.at[b]) for b in range(B)]
    ld_k, ld_v = {}, {}
    for slots in ((0, 1), (2, 5), (3, 4), (6, 7)):
        for src, dst, ld in ((k_hbm, k32, ld_k), (v_hbm, v32, ld_v)):
            for g in slots:
                owner = (me, left, right, diag)[g // 2]
                rows = pl.ds(pl.multiple_of((owner * 2 + g % 2) * LANES, LANES), LANES)
                ld[g] = load(src.at[pl.ds(me * B, B), rows], dst.at[g])

    @pl.when(me == 2)
    def _():
        pl.semaphore_wait(barrier, 2)
        for peer in (left, right):
            pl.semaphore_signal(ready, 1, device_id=(peer,), device_id_type=MESH)

    def first(buf, rows=slice(None)):
        return [remote(buf.at[0, rows], buf.at[2, rows], right),
                remote(buf.at[1, rows], buf.at[5, rows], left)]

    def second(buf, rows=slice(None)):
        return [remote(buf.at[1, rows], buf.at[3, rows], right),
                remote(buf.at[0, rows], buf.at[4, rows], left)]

    def forward(buf, rows=slice(None)):
        return [remote(buf.at[2, rows], buf.at[6, rows], right),
                remote(buf.at[5, rows], buf.at[7, rows], left)]

    def tile(n):
        return LOW_O + 32 * n

    rest = CUTS[-2] // 4
    early = [first(msg, slice(0, SUB))]
    early += [[remote(msg.at[0:2, a // 4:b // 4], msg.at[2:4, a // 4:b // 4], right),
               remote(msg.at[0:2, a // 4:b // 4], msg.at[4:6, a // 4:b // 4], left)]
              for a, b in pieces[1:-1]]
    early += [first(msg, slice(rest, PLANES_Q))]
    q1_planes = first(msg, slice(PLANES_Q, STREAM))
    q1_stream = first(msg, slice(STREAM, PLANES_O)) + first(top_q)
    q2 = second(msg, slice(rest, PLANES_O)) + second(top_q)
    o1_a = first(msg, slice(PLANES_O, tile(3)))
    o_tops = first(top_o) + second(top_o)
    qf = forward(msg, slice(LOW_Q, PLANES_O)) + forward(top_q)
    o1_b = first(msg, slice(tile(3), END))
    o2_a = second(msg, slice(PLANES_O, tile(1)))
    of_planes = forward(top_o) + forward(msg, slice(PLANES_O, LOW_O))
    o2_b = second(msg, slice(tile(1), tile(3)))
    o2_c = second(msg, slice(tile(3), END))
    of = [forward(msg, slice(tile(n), tile(n + 1))) for n in range(4)]

    peak = [[], []]
    for n, (a, b) in enumerate(pieces):
        loaded(ld_wq[n])
        words = [to_words(wq32[a:b, h * LANES:(h + 1) * LANES]) for h in range(2)]
        for h in range(2):
            msg[h, a // 4:b // 4] = cat(pack_low(vregs(words[h])))
        pl.when(me >= 2)(early[n][0].start)
        pl.when((me == 1) | (me == 2))(early[n][1].start)
        for h in range(2):
            w[h, a // 2:b // 2] = words[h]
            peak[h] = running_max(vregs(words[h]), peak[h])

    def encode(matrix, top):
        @pl.loop(0, 4)
        def _(i):
            h, j = i >> 1, 2 * matrix + (i & 1)
            rows = pl.ds(pl.multiple_of(j * 16 * SUB, 16 * SUB), 16 * SUB)
            parts[h, j] = cat(pack_high(vregs(w[h, rows]), top(h)))

    for h in range(2):
        top_q[h, 0] = column_max(peak[h])
    encode(0, lambda h: top_q[h, 0])
    for h in range(2):
        msg[h, PLANES_Q:STREAM] = cat(join_planes(vregs(parts[h, 0]), vregs(parts[h, 1])))

    @pl.when(me == 0)
    def _():
        pl.semaphore_wait(barrier, 2)

    @pl.when(odd)
    def _():
        pl.semaphore_wait(ready, 1)

    @pl.when(me < 2)
    def _():
        start([copies[0] for copies in early])

    @pl.when((me == 0) | (me == 3))
    def _():
        start([copies[1] for copies in early])

    start(q1_planes)
    pl.when(me != 3)(packed_head[0].start)
    pl.when(me != 1)(packed_head[1].start)

    for h in range(2):
        loaded(ld_wo[h])
        words = cat([to_words(wo32[h, :, n * LANES:(n + 1) * LANES]) for n in range(4)])
        w[h, WO:] = words
        msg[h, LOW_O:END] = cat(pack_low(vregs(words)))
        top_o[h] = column_max(running_max(vregs(words), []))
    encode(1, lambda h: top_o[h])
    for h in range(2):
        part = [vregs(parts[h, j]) for j in range(4)]
        bits, spare = join_runs([v[i:i + 2] for v in part for i in (4, 6)])
        msg[h, STREAM:LOW_O] = cat(bits + join_planes(part[2], part[3]))
        top_q[h, 1], top_q[h, 2] = spare
    start(q1_stream, q2, o1_a)

    stream, terms = {}, [0] * 4

    def decode_wq(g):
        bits = vregs(msg[g, STREAM:PLANES_O]) + [jnp.where(upper_sublanes(), top_q[g, 2], top_q[g, 1])]
        high, stream[g] = unpack_high(vregs(msg[g, PLANES_Q:STREAM]), top_q[g, 0], bits)
        return unpack_low(high, vregs(msg[g, LOW_Q:PLANES_Q]), top_q[g, 0])

    def decode_wo_high(g):
        return unpack_high(vregs(msg[g, PLANES_O:LOW_O]), top_o[g], stream[g])[0]

    def unpack_wq(*slots):
        for g in slots:
            w[g, :WO] = cat(decode_wq(g))

    def unpack_wo(*slots):
        for g in slots:
            w[g, WO:] = cat(decode_wo_high(g))

    def wo_tile(g, n):
        words = w[g, WO + BLK * n:WO + BLK * (n + 1)]
        if g >= 2:
            words = cat(unpack_low(vregs(words), vregs(msg[g, tile(n):tile(n + 1)]), top_o[g]))
        return to_bf16(words)

    def differences(decoded, words):
        return functools.reduce(jnp.bitwise_or, [a ^ b for a, b in zip(decoded, vregs(words))])

    def project_q(g, b=None, weights=w):
        rows = slice(None) if b is None else slice(b * S // 2, (b + 1) * S // 2)
        qbuf[g, rows] = to_words(jnp.dot(
            to_bf16(xb[rows]), to_bf16(weights[g, :WO]), preferred_element_type=F32))

    def keys(g):
        return [k32[g, b].astype(BF16).T for b in range(B)]

    def attend(g, p):
        for t in range(2):
            for b in range(B):
                ctx[g, (2 * b + t) * BLK:(2 * b + t + 1) * BLK] = context(*p[b], v32[g, b], t)

    def softmaxes(s):
        return [softmax(s[b]) for b in range(B)]

    def project_out(slots, *tiles):
        cols = slice(tiles[0] * LANES, (tiles[-1] + 1) * LANES)
        rhs = cat([jnp.concatenate([wo_tile(g, n) for n in tiles], 1) for g in slots])
        m = B * S * len(tiles) // 2
        for r in range(0, B * S, m):
            lhs = jnp.concatenate([to_bf16(ctx[g, r // 2:(r + m) // 2]) for g in slots], 1)
            res = jnp.dot(lhs, rhs, preferred_element_type=F32)
            if terms[tiles[0]] > 0:
                res = res + acc[r:r + m, cols]
            if terms[tiles[0]] == 3:
                out_ref[r:r + m, cols] = res.astype(out_ref.dtype)
            else:
                acc[r:r + m, cols] = res
        for n in tiles:
            terms[n] += 1

    loaded(ld_x[0])
    wrong = [differences(decode_wq(g), w[g, :WO]) for g in range(2)]
    xb[:S // 2] = to_words(x32[0] * SCALE)
    project_q(0, 0)
    project_q(1, 0)

    loaded(ld_x[1])
    for g in range(2):
        decoded = unpack_low(decode_wo_high(g), vregs(msg[g, LOW_O:END]), top_o[g])
        wrong[g] = differences(decoded, w[g, WO:]) | wrong[g]
        top_o[g] = top_o[g] | jnp.min(jnp.where(wrong[g] != 0, SIGN, 0), axis=0, keepdims=True)
    xb[S // 2:] = to_words(x32[1] * SCALE)
    project_q(0, 1)
    project_q(1, 1)

    loaded(ld_k[0], ld_k[1])
    s = [scores(qbuf[g], keys(g)) for g in range(2)]
    for g in range(2):
        for b, (e, inv) in enumerate(softmaxes(s[g])):
            pbuf[g, b] = cat(e + [jnp.broadcast_to(pltpu.bitcast(v, I32), (SUB, LANES)) for v in inv])

    loaded(ld_v[0], ld_v[1])
    start(o_tops)
    sent(*early, q1_planes)

    @pl.when(me == 0)
    def _():
        received(head)
        for j in range(2):
            msg[3 + j, 0:SUB] = cat(pack_low(vregs(to_words(head32[j]))))

    for j, sender in enumerate((3, 1)):
        pl.when(me == sender)(head[j].wait_send)
        pl.when(me != sender)(packed_head[j].wait_send)
        pl.when(me != 0)(packed_head[j].wait_recv)

    received(*early, q1_planes, q1_stream)
    start(qf, o1_b, o2_a)
    unpack_wq(2, 5)
    for g in range(2):
        attend(g, [([pbuf[g, b, P_ROWS[i]:P_ROWS[i + 1]] for i in range(NB)],
                    [pltpu.bitcast(pbuf[g, b, pl.ds(P_ROWS[NB] + SUB * i, 1)], F32) for i in range(NB)])
                   for b in range(B)])
    project_q(2)
    project_q(5)
    project_out((0, 1), 0)

    loaded(ld_k[2], ld_k[5], ld_v[2], ld_v[5])
    received(q2)
    unpack_wq(3, 4)
    project_out((0, 1), 1)
    s = scores(qbuf[2], keys(2))
    project_q(3)
    attend(2, softmaxes(s))
    s = scores(qbuf[5], keys(5))
    project_q(4, 0)
    attend(5, softmaxes(s))
    project_q(4, 1)

    loaded(ld_k[3], ld_k[4], ld_v[3], ld_v[4])
    received(o1_a, o_tops)
    start(of_planes, o2_b, o2_c, *of[:3])
    unpack_wo(2, 5)
    project_out((0, 1), 2)
    s = [scores(qbuf[g], keys(g)) for g in (3, 4)]
    project_out((0, 1), 3)
    attend(3, softmaxes(s[0]))
    attend(4, softmaxes(s[1]))
    project_out((2, 5), 0)

    loaded(ld_k[6], ld_k[7], ld_v[6], ld_v[7])
    sent(q1_stream, q2, o1_a, o_tops)
    received(qf)
    unpack_wq(6, 7)
    project_out((2, 5), 1, 2)
    project_q(6)
    project_q(7)
    for j in range(2):
        for b, k in enumerate(keys(6 + j)):
            kbuf[j, b] = pltpu.bitcast(k, I32)

    received(o1_b)
    start(of[3])
    received(o2_a)
    unpack_wo(3, 4)
    s = [scores(qbuf[6 + j], [to_bf16(kbuf[j, b]) for b in range(B)]) for j in range(2)]
    project_out((2, 5), 3)
    attend(6, softmaxes(s[0]))
    attend(7, softmaxes(s[1]))
    project_out((3, 4), 0)

    received(of_planes, o2_b)
    unpack_wo(6, 7)
    inexact = jnp.min(functools.reduce(jnp.bitwise_or, [top_o[g] for g in range(8)])) < 0
    project_out((3, 4), 1, 2)

    sent(qf, o1_b, o2_a, of_planes, o2_b)
    received(o2_c, of[0])
    project_out((3, 4), 3)
    project_out((6, 7), 0)
    for n in (1, 2):
        received(of[n])
        project_out((6, 7), n)
    sent(o2_c, *of)
    received(of[3])
    project_out((6, 7), 3)

    @pl.when(inexact)
    def _():
        plain[0:2] = w[0:2]
        gather = [first(plain), second(plain), forward(plain)]
        start(*gather[:2])
        received(gather[0])
        start(gather[2])
        acc[...] = jnp.zeros(acc.shape, F32)
        received(*gather[1:])
        sent(*gather)

        @pl.loop(0, 8)
        def _(g):
            project_q(g, weights=plain)
            attend(g, softmaxes(scores(qbuf[g], keys(g))))
            for n in range(4):
                acc[:, n * LANES:(n + 1) * LANES] += jnp.dot(
                    to_bf16(ctx[g]), to_bf16(plain[g, WO + BLK * n:WO + BLK * (n + 1)]),
                    preferred_element_type=F32)

        out_ref[...] = acc[...].astype(out_ref.dtype)


def pallas_dist_sparse_attn_causalblk_htp_bs_b2_sq256_skv256_hq4_dh64_kernel(
    x: jax.Array,
    Wq: jax.Array,
    K_ext: jax.Array,
    V_ext: jax.Array,
    Wo: jax.Array,
):
    batch, seq, heads, dim = K_ext.shape
    kt = jnp.transpose(K_ext, (0, 2, 3, 1)).reshape(batch, heads * dim, seq)
    vt = jnp.transpose(V_ext, (0, 2, 3, 1)).reshape(batch, heads * dim, seq)
    out = pl.pallas_call(
        kernel_body,
        out_shape=jax.ShapeDtypeStruct((B * S, D), BF16),
        in_specs=[pl.BlockSpec(memory_space=pl.ANY)] * 5,
        out_specs=pl.BlockSpec(memory_space=pltpu.VMEM),
        scratch_shapes=[
            pltpu.VMEM((D, 2 * LANES), F32),
            pltpu.VMEM((2, LANES, D), F32),
            pltpu.VMEM((B, S, D), F32),
            pltpu.VMEM((8, B, LANES, S), F32),
            pltpu.VMEM((8, B, LANES, S), F32),
            pltpu.VMEM((2, CUTS[1], LANES), F32),
            pltpu.VMEM((8, D, LANES), I32),
            pltpu.VMEM((8, D, LANES), I32),
            pltpu.VMEM((8, END, LANES), I32),
            pltpu.VMEM((8, 3, 1, LANES), I32),
            pltpu.VMEM((8, 1, LANES), I32),
            pltpu.VMEM((2, 4, 8 * SUB, LANES), I32),
            pltpu.VMEM((B * S // 2, D), I32),
            pltpu.VMEM((8, B * S // 2, LANES), I32),
            pltpu.VMEM((2, B, S // 2, LANES), I32),
            pltpu.VMEM((2, B, P_ROWS[NB] + NB * SUB, LANES), I32),
            pltpu.VMEM((8, B * S // 2, LANES), I32),
            pltpu.VMEM((B * S, D), F32),
            pltpu.SemaphoreType.DMA((25,)),
            pltpu.SemaphoreType.DMA((58,)),
            pltpu.SemaphoreType.DMA((58,)),
            pltpu.SemaphoreType.REGULAR,
        ],
        compiler_params=pltpu.CompilerParams(
            collective_id=0,
            vmem_limit_bytes=48 * 1024 * 1024,
            disable_semaphore_checks=True,
            flags={"XLA_TPU_FORCE_LP_LLO_SCHEDULER": True},
        ),
    )(x, Wq, kt, vt, Wo)
    return out.reshape(x.shape)
```

```python
import functools
import math

import jax
import jax.numpy as jnp
import numpy as np
from jax import lax
from jax.experimental import pallas as pl
from jax.experimental.pallas import tpu as pltpu

B = 2
S = 256
D = 512
BLK = 64
NB = S // BLK
LANES = 128
SUB = 8
SCALE = 0.125 * math.log2(math.e)
F32, BF16, I32 = jnp.float32, jnp.bfloat16, jnp.int32
MESH = pl.DeviceIdType.MESH

WO = D // 2
LOW_Q, PLANES_Q, STREAM, PLANES_O, LOW_O, END = 0, 128, 168, 184, 224, 352
CUTS = (0, 32, 64, 128, 224, D)
P_ROWS = (0, 32, 96, 192, 320)


def to_words(v):
    return pltpu.bitcast(v.astype(BF16), I32)


def to_bf16(v):
    return pltpu.bitcast(v, BF16)


def vregs(a):
    return [a[i:i + SUB] for i in range(0, a.shape[0], SUB)]


def cat(v):
    return jnp.concatenate(v, 0)


def _i32(v):
    return np.uint32(v).view(np.int32)


MAG, SIGN, BYTE, ONE = (_i32(v) for v in (0x7FFF7FFF, 0x80008000, 0x00FF00FF, 0x01000100))
RUN = 8
shl, shr = lax.shift_left, lax.shift_right_logical


def shift(x, n):
    if n == 0:
        return x
    return shl(x, np.int32(n)) if n > 0 else shr(x, np.int32(-n))


def upper_sublanes():
    return lax.broadcasted_iota(I32, (SUB, LANES), 0) >= SUB // 2


def pack_low(words):
    low = (words & BYTE).reshape(-1, 2, SUB, LANES)
    return (low[:, 0] | shift(low[:, 1], 8)).reshape(-1, LANES)


def running_max(words, acc=None):
    peak = [jnp.max((words & m).reshape(-1, SUB, LANES), axis=0) for m in (MAG, 0x7FFF)]
    return peak if acc is None else [jnp.maximum(a, b) for a, b in zip(acc, peak)]


def column_max(acc):
    hi, lo = (jnp.max(v, axis=0, keepdims=True) for v in acc)
    return (hi & _i32(0xFFFF0000)) | lo


def pack_high(words, top):
    top = jnp.broadcast_to(top, words[0].shape)
    fives, runs = [], []
    for k, a in enumerate(words):
        sign = a & SIGN if k == 0 else sign | shift(a & SIGN, -k)
        d = top - (a & MAG)
        classes = (shift(d, -8) & 0xFF, shift(d, -24))
        if k % RUN == 0:
            bits, pos = jnp.zeros_like(a), jnp.full_like(a, -1)
        if k < 15:
            far = shift((d + 0x7E007E00) & SIGN, -15)
            trit = far + shift((d + 0x7F007F00) & SIGN, -15)
            five = trit if k % 5 == 0 else five + shift(five, 1) + trit
            if k % 5 == 4:
                fives.append(five + (shift(five * 55 + 0x03FF03FF, -10) & 0x000F000F))
            for c, e in zip(classes, (far & 1, shift(far, -16))):
                pos = pos + ((c - 1) & -e)
                bits = bits | shl(e, pos & 31)
        else:
            for c in classes:
                pos = pos + c + 1
                bits = bits | shl(jnp.ones_like(a), pos & 31)
        if k % RUN == RUN - 1:
            runs += [bits, (pos + 1) & 31]
    return [sign] + fives + runs


def join_planes(a, b):
    return [a[0], b[0]] + [a[j] | shift(b[j], 8) for j in (1, 2, 3)]


def join_runs(runs):
    r = [runs[-1][0]] + [jnp.zeros_like(runs[0][0])] * 2
    for bits, n in reversed(runs[:-1]):
        r = [shl(r[0], n) | bits] + [shl(r[i], n) | shr(shift(r[i - 1], -1), 31 - n) for i in (1, 2)]
    spare = [jnp.sum(jnp.where(upper_sublanes(), 0, r[2]), axis=0, keepdims=True),
             jnp.sum(jnp.where(upper_sublanes(), r[2], 0), axis=0, keepdims=True)]
    return r[:2], spare


def unpack_high(planes, top, r):
    signs, x = planes[:, :2 * SUB], planes[:, 2 * SUB:]
    top = jnp.broadcast_to(top & MAG, r[0].shape)
    x = jnp.concatenate([x, shift(x, -8)], 1)
    trits = []
    for _ in range(5):
        x = x & BYTE
        x = x + shift(x, 1)
        trits.append(((x | shift(x, -1)) & ONE, shift(x, -9) & 1, shift(x, -25)))
    signs = [shift(signs, k) & SIGN for k in range(16)]
    out = []
    for run in range(0, 32, RUN):
        bits, base, counts = r[0], [], ([], [])
        for k in range(run, run + RUN):
            half, j = divmod(k, 16)
            if j < 15:
                at = (3 * half + j // 5) * SUB
                near, *unary = (v[:, at:at + SUB] for v in trits[j % 5])
            else:
                near, unary = -ONE, (1, 1)
            base.append(top - near + signs[j][:, half * SUB:(half + 1) * SUB])
            for count, e in zip(counts, unary):
                count.append(lax.population_count(bits ^ (bits - e)))
                bits = shr(bits, count[-1])
        extra = shift(jnp.concatenate(counts[0], 1), 8) + shift(jnp.concatenate(counts[1], 1), 24)
        out.append(jnp.concatenate(base, 1) - extra)
        used = jnp.sum(extra.reshape(-1, RUN, SUB, LANES), axis=1)
        n = (shift(used, -8) + shift(used, -24)) & 31
        r = [bits | shl(shift(r[1], 1), 31 - n),
             shr(r[1], n) | shl(shift(r[2], 1), 31 - n),
             shr(r[2], n)]
    return jnp.concatenate(out, 1), r


def unpack_low(high, low, top):
    low = low.reshape(-1, 1, SUB, LANES)
    low = jnp.concatenate([low, shift(low, -8)], 1).reshape(high.shape) & BYTE
    return high - (((top | ONE) - low) & BYTE)


def first_half(rows):
    return lax.broadcasted_iota(I32, (rows, LANES), 1) < BLK


def scores(q, k):
    h = BLK // 2
    out = [[None] * NB for _ in range(B)]
    for qb in reversed(range(NB)):
        for b in range(B):
            block = q[(b * NB + qb) * h:(b * NB + qb + 1) * h]
            h0, h1 = jnp.where(first_half(h), block, 0), jnp.where(first_half(h), 0, block)
            rhs = to_bf16(cat([h0, h1] if qb % 2 == 0 else [h1, h0]))
            out[b][qb] = lax.dot_general(
                k[b][:(qb + 1) * BLK], rhs, (((1,), (1,)), ((), ())), preferred_element_type=F32)
    return out


def softmax(s):
    e = [jnp.exp2(v - jnp.max(v, axis=0, keepdims=True)) for v in s]
    total = [jnp.sum(v, axis=0, keepdims=True) for v in e]
    inv = [1.0 / v for v in total]
    return [to_words(v) for v in e], inv


def context(e, inv, vt, t):
    h = BLK // 2
    a, b = e[2 * t], e[2 * t + 1]
    n = a.shape[0]
    p0 = to_bf16(cat([jnp.where(first_half(n), a, b[:n]), jnp.where(first_half(h), 0, b[n:])]))
    p1 = to_bf16(cat([jnp.where(first_half(n), b[:n], a), jnp.where(first_half(h), b[n:], 0)]))
    keys = p0.shape[0]
    c0 = jnp.dot(vt[:BLK, :keys].astype(BF16), p0, preferred_element_type=F32)
    c1 = jnp.dot(vt[BLK:, :keys].astype(BF16), p1, preferred_element_type=F32)
    c0 = c0 * jnp.where(first_half(1), inv[2 * t], inv[2 * t + 1])
    c1 = c1 * jnp.where(first_half(1), inv[2 * t + 1], inv[2 * t])
    c = pltpu.bitcast(cat([c0, c1]).astype(BF16).T, I32)
    return cat([jnp.where(first_half(h), c[:h], c[h:]), jnp.where(first_half(h), c[h:], c[:h])])


def kernel_body(x_hbm, wq_hbm, k_hbm, v_hbm, wo_hbm, out_ref,
                wq32, wo32, x32, k32, v32, head32,
                w, plain, msg, top_q, top_o, parts,
                xb, qbuf, kbuf, pbuf, ctx, acc,
                load_sem, send_sem, recv_sem, ready):
    load_ids = iter(range(load_sem.shape[0]))
    copy_ids = iter(range(6, send_sem.shape[0]))

    def load(src, dst):
        copy = pltpu.make_async_copy(src, dst, load_sem.at[next(load_ids)])
        copy.start()
        return copy

    def remote(src, dst, to, send=None, recv=None):
        recv = next(copy_ids) if recv is None else recv
        send = recv if send is None else send
        return pltpu.make_async_remote_copy(
            src, dst, send_sem.at[send], recv_sem.at[recv], device_id=(to,), device_id_type=MESH)

    def start(*groups):
        for group in groups:
            for copy in group:
                copy.start()

    def received(*groups):
        for group in groups:
            for copy in group:
                copy.wait_recv()

    def sent(*groups):
        for group in groups:
            for copy in group:
                copy.wait_send()

    def loaded(*copies):
        for copy in copies:
            copy.wait()

    pieces = tuple(zip(CUTS[:-1], CUTS[1:]))
    ld_wq = [load(wq_hbm.at[a:b], wq32.at[a:b]) for a, b in pieces]

    me = lax.axis_index("i")
    left, right, diag = (me + 3) & 3, (me + 1) & 3, me ^ 2
    odd = (me & 1) == 1

    barrier = pltpu.get_barrier_semaphore()
    head = [remote(wq_hbm.at[0:CUTS[1], LANES:], head32.at[0], right, recv=0),
            remote(wq_hbm.at[0:CUTS[1], :LANES], head32.at[1], left, recv=1)]
    packed_head = [remote(msg.at[1, 0:SUB], msg.at[3, 0:SUB], right, recv=0),
                   remote(msg.at[0, 0:SUB], msg.at[4, 0:SUB], left, recv=1)]

    @pl.when(me != 2)
    def _():
        for peer in (left, right):
            pl.semaphore_signal(barrier, 1, device_id=(peer,), device_id_type=MESH)

    @pl.when(odd)
    def _():
        pl.semaphore_wait(barrier, 1)
        pl.when(me == 3)(head[0].start)
        pl.when(me == 1)(head[1].start)

    ld_wo = [load(wo_hbm.at[h * LANES:(h + 1) * LANES], wo32.at[h]) for h in range(2)]
    ld_x = [load(x_hbm.at[b], x32.at[b]) for b in range(B)]
    ld_k, ld_v = {}, {}
    for slots in ((0, 1), (2, 5), (3, 4), (6, 7)):
        for src, dst, ld in ((k_hbm, k32, ld_k), (v_hbm, v32, ld_v)):
            for g in slots:
                owner = (me, left, right, diag)[g // 2]
                rows = pl.ds(pl.multiple_of((owner * 2 + g % 2) * LANES, LANES), LANES)
                ld[g] = load(src.at[pl.ds(me * B, B), rows], dst.at[g])

    @pl.when(me == 2)
    def _():
        pl.semaphore_wait(barrier, 2)
        for peer in (left, right):
            pl.semaphore_signal(ready, 1, device_id=(peer,), device_id_type=MESH)

    def first(buf, rows=slice(None), send=(None, None)):
        return [remote(buf.at[0, rows], buf.at[2, rows], right, send[0]),
                remote(buf.at[1, rows], buf.at[5, rows], left, send[1])]

    def second(buf, rows=slice(None), send=(None, None)):
        return [remote(buf.at[1, rows], buf.at[3, rows], right, send[0]),
                remote(buf.at[0, rows], buf.at[4, rows], left, send[1])]

    def forward(buf, rows=slice(None), send=(None, None)):
        return [remote(buf.at[2, rows], buf.at[6, rows], right, send[0]),
                remote(buf.at[5, rows], buf.at[7, rows], left, send[1])]

    def tile(n):
        return LOW_O + 32 * n

    rest = CUTS[-2] // 4
    early = [first(msg, slice(0, SUB))]
    early += [[remote(msg.at[0:2, a // 4:b // 4], msg.at[2:4, a // 4:b // 4], right),
               remote(msg.at[0:2, a // 4:b // 4], msg.at[4:6, a // 4:b // 4], left)]
              for a, b in pieces[1:-1]]
    early += [first(msg, slice(rest, PLANES_Q))]
    q1_planes = first(msg, slice(PLANES_Q, STREAM))
    q1_stream = first(msg, slice(STREAM, PLANES_O)) + first(top_q)
    q2 = second(msg, slice(rest, PLANES_O)) + second(top_q)
    o_tops = first(top_o) + second(top_o)
    qf_top, of_top = forward(top_q), forward(top_o)
    o1_a = first(msg, slice(PLANES_O, tile(3)), (2, 3))
    o1_b = first(msg, slice(tile(3), END), (2, 3))
    o2_a = second(msg, slice(PLANES_O, tile(1)), (2, 3))
    o2_b = second(msg, slice(tile(1), tile(3)), (2, 3))
    o2_c = second(msg, slice(tile(3), END), (2, 3))
    o_all = [remote(msg.at[0:2, PLANES_O:], msg.at[2:4, PLANES_O:], right, 2, 2),
             remote(msg.at[0:2, PLANES_O:], msg.at[4:6, PLANES_O:], left, 3, 3)]
    qf = forward(msg, slice(LOW_Q, PLANES_O), (4, 5))
    of_planes = forward(msg, slice(PLANES_O, LOW_O), (4, 5))
    of = [forward(msg, slice(tile(n), tile(n + 1)), (4, 5)) for n in range(4)]
    f_all = [remote(msg.at[2], msg.at[6], right, 4, 4), remote(msg.at[5], msg.at[7], left, 5, 5)]

    peak = [None, None]
    for n, (a, b) in enumerate(pieces):
        loaded(ld_wq[n])
        words = [to_words(wq32[a:b, h * LANES:(h + 1) * LANES]) for h in range(2)]
        for h in range(2):
            msg[h, a // 4:b // 4] = pack_low(words[h])
        pl.when(me >= 2)(early[n][0].start)
        pl.when((me == 1) | (me == 2))(early[n][1].start)
        for h in range(2):
            w[h, a // 2:b // 2] = words[h]
            peak[h] = running_max(words[h], peak[h])

    def encode(matrix, top):
        @pl.loop(0, 4)
        def _(i):
            h, j = i >> 1, 2 * matrix + (i & 1)
            rows = pl.ds(pl.multiple_of(j * 16 * SUB, 16 * SUB), 16 * SUB)
            parts[h, j] = cat(pack_high(vregs(w[h, rows]), top(h)))

    for h in range(2):
        top_q[h, 0] = column_max(peak[h])
    encode(0, lambda h: top_q[h, 0])
    for h in range(2):
        msg[h, PLANES_Q:STREAM] = cat(join_planes(vregs(parts[h, 0]), vregs(parts[h, 1])))

    @pl.when(me == 0)
    def _():
        pl.semaphore_wait(barrier, 2)

    @pl.when(odd)
    def _():
        pl.semaphore_wait(ready, 1)

    @pl.when(me < 2)
    def _():
        start([copies[0] for copies in early])

    @pl.when((me == 0) | (me == 3))
    def _():
        start([copies[1] for copies in early])

    start(q1_planes)
    pl.when(me != 3)(packed_head[0].start)
    pl.when(me != 1)(packed_head[1].start)

    for h in range(2):
        loaded(ld_wo[h])
        words = cat([to_words(wo32[h, :, n * LANES:(n + 1) * LANES]) for n in range(4)])
        w[h, WO:] = words
        msg[h, LOW_O:END] = pack_low(words)
        top_o[h] = column_max(running_max(words))
    encode(1, lambda h: top_o[h])
    for h in range(2):
        part = [vregs(parts[h, j]) for j in range(4)]
        bits, spare = join_runs([v[i:i + 2] for v in part for i in (4, 6)])
        msg[h, STREAM:LOW_O] = cat(bits + join_planes(part[2], part[3]))
        top_q[h, 1], top_q[h, 2] = spare
    start(q1_stream, q2, o1_a)

    stream, terms = {}, [0] * 4

    def gather(ref, slots, at):
        return cat([ref[g:g + 1, at] for g in slots])

    def decode_wq(*slots):
        spare = [jnp.where(upper_sublanes(), top_q[g, 2], top_q[g, 1])[None] for g in slots]
        bits = [gather(msg, slots, pl.ds(STREAM + i * SUB, SUB)) for i in range(2)] + [cat(spare)]
        high, stream[slots] = unpack_high(
            gather(msg, slots, slice(PLANES_Q, STREAM)), gather(top_q, slots, 0), bits)
        return [unpack_low(high[j], msg[g, LOW_Q:PLANES_Q], top_q[g, 0]) for j, g in enumerate(slots)]

    def decode_wo_high(*slots):
        high, _ = unpack_high(
            gather(msg, slots, slice(PLANES_O, LOW_O)), gather(top_o, slots, slice(None)), stream[slots])
        return [high[j] for j in range(len(slots))]

    def unpack_wq(*slots):
        for g, words in zip(slots, decode_wq(*slots)):
            w[g, :WO] = words

    def unpack_wo(*slots):
        for g, high in zip(slots, decode_wo_high(*slots)):
            w[g, WO:] = high

    def wo_tile(g, n):
        words = w[g, WO + BLK * n:WO + BLK * (n + 1)]
        if g >= 2:
            words = unpack_low(words, msg[g, tile(n):tile(n + 1)], top_o[g])
        return to_bf16(words)

    def differences(decoded, words):
        return functools.reduce(jnp.bitwise_or, vregs(decoded ^ words))

    def project_q(g, b=None, weights=w):
        rows = slice(None) if b is None else slice(b * S // 2, (b + 1) * S // 2)
        qbuf[g, rows] = to_words(jnp.dot(
            to_bf16(xb[rows]), to_bf16(weights[g, :WO]), preferred_element_type=F32))

    def keys(g):
        return [k32[g, b].astype(BF16).T for b in range(B)]

    def attend(g, p):
        for t in range(2):
            for b in range(B):
                ctx[g, (2 * b + t) * BLK:(2 * b + t + 1) * BLK] = context(*p[b], v32[g, b], t)

    def softmaxes(s):
        return [softmax(s[b]) for b in range(B)]

    def project_out(slots, *tiles):
        cols = slice(tiles[0] * LANES, (tiles[-1] + 1) * LANES)
        rhs = cat([jnp.concatenate([wo_tile(g, n) for n in tiles], 1) for g in slots])
        m = B * S * len(tiles) // 2
        for r in range(0, B * S, m):
            lhs = jnp.concatenate([to_bf16(ctx[g, r // 2:(r + m) // 2]) for g in slots], 1)
            res = jnp.dot(lhs, rhs, preferred_element_type=F32)
            if terms[tiles[0]] > 0:
                res = res + acc[r:r + m, cols]
            if terms[tiles[0]] == 3:
                out_ref[r:r + m, cols] = res.astype(out_ref.dtype)
            else:
                acc[r:r + m, cols] = res
        for n in tiles:
            terms[n] += 1

    loaded(ld_x[0])
    wrong = [differences(decoded, w[g, :WO]) for g, decoded in enumerate(decode_wq(0, 1))]
    xb[:S // 2] = to_words(x32[0] * SCALE)
    project_q(0, 0)
    project_q(1, 0)

    loaded(ld_x[1])
    for g, high in enumerate(decode_wo_high(0, 1)):
        decoded = unpack_low(high, msg[g, LOW_O:END], top_o[g])
        wrong[g] = differences(decoded, w[g, WO:]) | wrong[g]
        top_o[g] = top_o[g] | jnp.min(jnp.where(wrong[g] != 0, SIGN, 0), axis=0, keepdims=True)
    xb[S // 2:] = to_words(x32[1] * SCALE)
    project_q(0, 1)
    project_q(1, 1)

    loaded(ld_k[0], ld_k[1])
    s = [scores(qbuf[g], keys(g)) for g in range(2)]
    for g in range(2):
        for b, (e, inv) in enumerate(softmaxes(s[g])):
            pbuf[g, b] = cat(e + [jnp.broadcast_to(pltpu.bitcast(v, I32), (SUB, LANES)) for v in inv])

    loaded(ld_v[0], ld_v[1])
    start(o_tops)
    sent(*early, q1_planes)

    @pl.when(me == 0)
    def _():
        received(head)
        for j in range(2):
            msg[3 + j, 0:SUB] = pack_low(to_words(head32[j]))

    for j, sender in enumerate((3, 1)):
        pl.when(me == sender)(head[j].wait_send)
        pl.when(me != sender)(packed_head[j].wait_send)
        pl.when(me != 0)(packed_head[j].wait_recv)

    received(*early, q1_planes, q1_stream)
    start(qf_top, qf, o1_b, o2_a)
    unpack_wq(2, 5)
    for g in range(2):
        attend(g, [([pbuf[g, b, P_ROWS[i]:P_ROWS[i + 1]] for i in range(NB)],
                    [pltpu.bitcast(pbuf[g, b, pl.ds(P_ROWS[NB] + SUB * i, 1)], F32) for i in range(NB)])
                   for b in range(B)])
    project_q(2)
    project_q(5)
    project_out((0, 1), 0)

    loaded(ld_k[2], ld_k[5], ld_v[2], ld_v[5])
    received(q2)
    unpack_wq(3, 4)
    project_out((0, 1), 1)
    s = scores(qbuf[2], keys(2))
    project_q(3)
    attend(2, softmaxes(s))
    s = scores(qbuf[5], keys(5))
    project_q(4, 0)
    attend(5, softmaxes(s))
    project_q(4, 1)

    loaded(ld_k[3], ld_k[4], ld_v[3], ld_v[4])
    received(o1_a, o_tops)
    start(of_top, of_planes, o2_b, o2_c, *of[:3])
    unpack_wo(2, 5)
    project_out((0, 1), 2)
    s = [scores(qbuf[g], keys(g)) for g in (3, 4)]
    project_out((0, 1), 3)
    attend(3, softmaxes(s[0]))
    attend(4, softmaxes(s[1]))
    project_out((2, 5), 0)

    loaded(ld_k[6], ld_k[7], ld_v[6], ld_v[7])
    sent(q1_stream, q2, o_tops, qf_top)
    received(qf_top, qf)
    unpack_wq(6, 7)
    project_out((2, 5), 1, 2)
    project_q(6)
    project_q(7)
    for j in range(2):
        for b, k in enumerate(keys(6 + j)):
            kbuf[j, b] = pltpu.bitcast(k, I32)

    received(o1_b)
    start(of[3])
    received(o2_a)
    unpack_wo(3, 4)
    s = [scores(qbuf[6 + j], [to_bf16(kbuf[j, b]) for b in range(B)]) for j in range(2)]
    project_out((2, 5), 3)
    attend(6, softmaxes(s[0]))
    attend(7, softmaxes(s[1]))
    project_out((3, 4), 0)

    received(of_top, of_planes, o2_b)
    unpack_wo(6, 7)
    inexact = jnp.min(functools.reduce(jnp.bitwise_or, [top_o[g] for g in range(8)])) < 0
    project_out((3, 4), 1, 2)

    sent(of_top)
    received(o2_c, of[0])
    project_out((3, 4), 3)
    project_out((6, 7), 0)
    for n in (1, 2):
        received(of[n])
        project_out((6, 7), n)
    sent(o_all, f_all)
    received(of[3])
    project_out((6, 7), 3)

    @pl.when(inexact)
    def _():
        plain[0:2] = w[0:2]
        copies = [first(plain), second(plain), forward(plain)]
        start(*copies[:2])
        received(copies[0])
        start(copies[2])
        acc[...] = jnp.zeros(acc.shape, F32)
        received(*copies[1:])
        sent(*copies)

        @pl.loop(0, 8)
        def _(g):
            project_q(g, weights=plain)
            attend(g, softmaxes(scores(qbuf[g], keys(g))))
            for n in range(4):
                acc[:, n * LANES:(n + 1) * LANES] += jnp.dot(
                    to_bf16(ctx[g]), to_bf16(plain[g, WO + BLK * n:WO + BLK * (n + 1)]),
                    preferred_element_type=F32)

        out_ref[...] = acc[...].astype(out_ref.dtype)


def pallas_dist_sparse_attn_causalblk_htp_bs_b2_sq256_skv256_hq4_dh64_kernel(
    x: jax.Array,
    Wq: jax.Array,
    K_ext: jax.Array,
    V_ext: jax.Array,
    Wo: jax.Array,
):
    batch, seq, heads, dim = K_ext.shape
    kt = jnp.transpose(K_ext, (0, 2, 3, 1)).reshape(batch, heads * dim, seq)
    vt = jnp.transpose(V_ext, (0, 2, 3, 1)).reshape(batch, heads * dim, seq)
    out = pl.pallas_call(
        kernel_body,
        out_shape=jax.ShapeDtypeStruct((B * S, D), BF16),
        in_specs=[pl.BlockSpec(memory_space=pl.ANY)] * 5,
        out_specs=pl.BlockSpec(memory_space=pltpu.VMEM),
        scratch_shapes=[
            pltpu.VMEM((D, 2 * LANES), F32),
            pltpu.VMEM((2, LANES, D), F32),
            pltpu.VMEM((B, S, D), F32),
            pltpu.VMEM((8, B, LANES, S), F32),
            pltpu.VMEM((8, B, LANES, S), F32),
            pltpu.VMEM((2, CUTS[1], LANES), F32),
            pltpu.VMEM((8, D, LANES), I32),
            pltpu.VMEM((8, D, LANES), I32),
            pltpu.VMEM((8, END, LANES), I32),
            pltpu.VMEM((8, 3, 1, LANES), I32),
            pltpu.VMEM((8, 1, LANES), I32),
            pltpu.VMEM((2, 4, 8 * SUB, LANES), I32),
            pltpu.VMEM((B * S // 2, D), I32),
            pltpu.VMEM((8, B * S // 2, LANES), I32),
            pltpu.VMEM((2, B, S // 2, LANES), I32),
            pltpu.VMEM((2, B, P_ROWS[NB] + NB * SUB, LANES), I32),
            pltpu.VMEM((8, B * S // 2, LANES), I32),
            pltpu.VMEM((B * S, D), F32),
            pltpu.SemaphoreType.DMA((25,)),
            pltpu.SemaphoreType.DMA((62,)),
            pltpu.SemaphoreType.DMA((62,)),
            pltpu.SemaphoreType.REGULAR,
        ],
        compiler_params=pltpu.CompilerParams(
            collective_id=0,
            vmem_limit_bytes=48 * 1024 * 1024,
            disable_semaphore_checks=True,
            flags={"XLA_TPU_FORCE_LP_LLO_SCHEDULER": True},
        ),
    )(x, Wq, kt, vt, Wo)
    return out.reshape(x.shape)
```

```python
import functools
import math

import jax
import jax.numpy as jnp
import numpy as np
from jax import lax
from jax.experimental import pallas as pl
from jax.experimental.pallas import tpu as pltpu

B = 2
S = 256
D = 512
BLK = 64
NB = S // BLK
LANES = 128
SUB = 8
SCALE = 0.125 * math.log2(math.e)
F32, BF16, I32 = jnp.float32, jnp.bfloat16, jnp.int32
MESH = pl.DeviceIdType.MESH

WO = D // 2
LOW_Q, PLANES_Q, STREAM, PLANES_O, LOW_O, END = 0, 128, 168, 184, 224, 352
CUTS = (0, 32, 64, 128, 224, D)
P_ROWS = (0, 32, 96, 192, 320)


def to_words(v):
    return pltpu.bitcast(v.astype(BF16), I32)


def to_bf16(v):
    return pltpu.bitcast(v, BF16)


def vregs(a):
    return [a[i:i + SUB] for i in range(0, a.shape[0], SUB)]


def cat(v):
    return jnp.concatenate(v, 0)


def _i32(v):
    return np.uint32(v).view(np.int32)


MAG, SIGN, BYTE, ONE = (_i32(v) for v in (0x7FFF7FFF, 0x80008000, 0x00FF00FF, 0x01000100))
RUN = 8
shl, shr = lax.shift_left, lax.shift_right_logical


def shift(x, n):
    if n == 0:
        return x
    return shl(x, np.int32(n)) if n > 0 else shr(x, np.int32(-n))


def upper_sublanes():
    return lax.broadcasted_iota(I32, (SUB, LANES), 0) >= SUB // 2


def pack_low(words):
    low = (words & BYTE).reshape(-1, 2, SUB, LANES)
    return (low[:, 0] | shift(low[:, 1], 8)).reshape(-1, LANES)


def running_max(words, acc=None):
    peak = [jnp.max((words & m).reshape(-1, SUB, LANES), axis=0) for m in (MAG, 0x7FFF)]
    return peak if acc is None else [jnp.maximum(a, b) for a, b in zip(acc, peak)]


def column_max(acc):
    hi, lo = (jnp.max(v, axis=0, keepdims=True) for v in acc)
    return (hi & _i32(0xFFFF0000)) | lo


def pack_high(words, top):
    top = jnp.broadcast_to(top, words[0].shape)
    fives, runs = [], []
    for k, a in enumerate(words):
        sign = a & SIGN if k == 0 else sign | shift(a & SIGN, -k)
        d = top - (a & MAG)
        classes = (shift(d, -8) & 0xFF, shift(d, -24))
        if k % RUN == 0:
            bits, pos = jnp.zeros_like(a), jnp.full_like(a, -1)
        if k < 15:
            far = shift((d + 0x7E007E00) & SIGN, -15)
            trit = far + shift((d + 0x7F007F00) & SIGN, -15)
            five = trit if k % 5 == 0 else five + shift(five, 1) + trit
            if k % 5 == 4:
                fives.append(five + (shift(five * 55 + 0x03FF03FF, -10) & 0x000F000F))
            for c, e in zip(classes, (far & 1, shift(far, -16))):
                pos = pos + ((c - 1) & -e)
                bits = bits | shl(e, pos & 31)
        else:
            for c in classes:
                pos = pos + c + 1
                bits = bits | shl(jnp.ones_like(a), pos & 31)
        if k % RUN == RUN - 1:
            runs += [bits, (pos + 1) & 31]
    return [sign] + fives + runs


def join_planes(a, b):
    return [a[0], b[0]] + [a[j] | shift(b[j], 8) for j in (1, 2, 3)]


def join_runs(runs):
    r = [runs[-1][0]] + [jnp.zeros_like(runs[0][0])] * 2
    for bits, n in reversed(runs[:-1]):
        r = [shl(r[0], n) | bits] + [shl(r[i], n) | shr(shift(r[i - 1], -1), 31 - n) for i in (1, 2)]
    spare = [jnp.sum(jnp.where(upper_sublanes(), 0, r[2]), axis=0, keepdims=True),
             jnp.sum(jnp.where(upper_sublanes(), r[2], 0), axis=0, keepdims=True)]
    return r[:2], spare


def unpack_high(planes, top, r):
    signs, x = planes[:, :2 * SUB], planes[:, 2 * SUB:]
    top = jnp.broadcast_to(top & MAG, r[0].shape)
    x = jnp.concatenate([x, shift(x, -8)], 1)
    trits = []
    for _ in range(5):
        x = x & BYTE
        x = x + shift(x, 1)
        trits.append(((x | shift(x, -1)) & ONE, shift(x, -9) & 1, shift(x, -25)))
    signs = [shift(signs, k) & SIGN for k in range(16)]
    out = []
    for run in range(0, 32, RUN):
        bits, base, counts = r[0] | _i32(0xC0000000), [], ([], [])
        for k in range(run, run + RUN):
            half, j = divmod(k, 16)
            if j < 15:
                at = (3 * half + j // 5) * SUB
                near, *unary = (v[:, at:at + SUB] for v in trits[j % 5])
            else:
                near, unary = -ONE, (1, 1)
            base.append(top - near + signs[j][:, half * SUB:(half + 1) * SUB])
            for count, e in zip(counts, unary):
                count.append(lax.population_count(bits ^ (bits - e)))
                bits = lax.shift_right_arithmetic(bits, count[-1])
        extra = shift(jnp.concatenate(counts[0], 1), 8) + shift(jnp.concatenate(counts[1], 1), 24)
        out.append(jnp.concatenate(base, 1) - extra)
        used = jnp.sum(extra.reshape(-1, RUN, SUB, LANES), axis=1)
        n = (shift(used, -8) + shift(used, -24)) & 31
        r = [shr(r[i], n) | shl(shift(r[i + 1], 1), 31 - n) for i in range(2)] + [shr(r[2], n)]
    return jnp.concatenate(out, 1), r


def unpack_low(high, low, top):
    low = low.reshape(-1, 1, SUB, LANES)
    low = jnp.concatenate([low, shift(low, -8)], 1).reshape(high.shape) & BYTE
    return high - (((top | ONE) - low) & BYTE)


def first_half(rows):
    return lax.broadcasted_iota(I32, (rows, LANES), 1) < BLK


def scores(q, k):
    h = BLK // 2
    out = [[None] * NB for _ in range(B)]
    for qb in reversed(range(NB)):
        for b in range(B):
            block = q[(b * NB + qb) * h:(b * NB + qb + 1) * h]
            h0, h1 = jnp.where(first_half(h), block, 0), jnp.where(first_half(h), 0, block)
            rhs = to_bf16(cat([h0, h1] if qb % 2 == 0 else [h1, h0]))
            out[b][qb] = lax.dot_general(
                k[b][:(qb + 1) * BLK], rhs, (((1,), (1,)), ((), ())), preferred_element_type=F32)
    return out


def softmax(s):
    e = [jnp.exp2(v - jnp.max(v, axis=0, keepdims=True)) for v in s]
    total = [jnp.sum(v, axis=0, keepdims=True) for v in e]
    inv = [1.0 / v for v in total]
    return [to_words(v) for v in e], inv


def context(e, inv, vt, t):
    h = BLK // 2
    a, b = e[2 * t], e[2 * t + 1]
    n = a.shape[0]
    p0 = to_bf16(cat([jnp.where(first_half(n), a, b[:n]), jnp.where(first_half(h), 0, b[n:])]))
    p1 = to_bf16(cat([jnp.where(first_half(n), b[:n], a), jnp.where(first_half(h), b[n:], 0)]))
    keys = p0.shape[0]
    c0 = jnp.dot(vt[:BLK, :keys].astype(BF16), p0, preferred_element_type=F32)
    c1 = jnp.dot(vt[BLK:, :keys].astype(BF16), p1, preferred_element_type=F32)
    c0 = c0 * jnp.where(first_half(1), inv[2 * t], inv[2 * t + 1])
    c1 = c1 * jnp.where(first_half(1), inv[2 * t + 1], inv[2 * t])
    c = pltpu.bitcast(cat([c0, c1]).astype(BF16).T, I32)
    return cat([jnp.where(first_half(h), c[:h], c[h:]), jnp.where(first_half(h), c[h:], c[:h])])


def kernel_body(x_hbm, wq_hbm, k_hbm, v_hbm, wo_hbm, out_ref,
                wq32, wo32, x32, k32, v32, head32,
                w, plain, msg, top_q, top_o, parts,
                xb, qbuf, kbuf, pbuf, ctx, acc,
                load_sem, send_sem, recv_sem, ready):
    load_ids = iter(range(load_sem.shape[0]))
    copy_ids = iter(range(6, send_sem.shape[0]))

    def load(src, dst):
        copy = pltpu.make_async_copy(src, dst, load_sem.at[next(load_ids)])
        copy.start()
        return copy

    def remote(src, dst, to, send=None, recv=None):
        recv = next(copy_ids) if recv is None else recv
        send = recv if send is None else send
        return pltpu.make_async_remote_copy(
            src, dst, send_sem.at[send], recv_sem.at[recv], device_id=(to,), device_id_type=MESH)

    def start(*groups):
        for group in groups:
            for copy in group:
                copy.start()

    def received(*groups):
        for group in groups:
            for copy in group:
                copy.wait_recv()

    def sent(*groups):
        for group in groups:
            for copy in group:
                copy.wait_send()

    def loaded(*copies):
        for copy in copies:
            copy.wait()

    pieces = tuple(zip(CUTS[:-1], CUTS[1:]))
    ld_wq = [load(wq_hbm.at[a:b], wq32.at[a:b]) for a, b in pieces]

    me = lax.axis_index("i")
    left, right, diag = (me + 3) & 3, (me + 1) & 3, me ^ 2
    odd = (me & 1) == 1

    barrier = pltpu.get_barrier_semaphore()
    head = [remote(wq_hbm.at[0:CUTS[1], LANES:], head32.at[0], right, recv=0),
            remote(wq_hbm.at[0:CUTS[1], :LANES], head32.at[1], left, recv=1)]
    packed_head = [remote(msg.at[1, 0:SUB], msg.at[3, 0:SUB], right, recv=0),
                   remote(msg.at[0, 0:SUB], msg.at[4, 0:SUB], left, recv=1)]

    @pl.when(me != 2)
    def _():
        for peer in (left, right):
            pl.semaphore_signal(barrier, 1, device_id=(peer,), device_id_type=MESH)

    @pl.when(odd)
    def _():
        pl.semaphore_wait(barrier, 1)
        pl.when(me == 3)(head[0].start)
        pl.when(me == 1)(head[1].start)

    ld_wo = [load(wo_hbm.at[h * LANES:(h + 1) * LANES], wo32.at[h]) for h in range(2)]
    ld_x = [load(x_hbm.at[b], x32.at[b]) for b in range(B)]
    ld_k, ld_v = {}, {}
    for slots in ((0, 1), (2, 5), (3, 4), (6, 7)):
        for src, dst, ld in ((k_hbm, k32, ld_k), (v_hbm, v32, ld_v)):
            for g in slots:
                owner = (me, left, right, diag)[g // 2]
                rows = pl.ds(pl.multiple_of((owner * 2 + g % 2) * LANES, LANES), LANES)
                ld[g] = load(src.at[pl.ds(me * B, B), rows], dst.at[g])

    @pl.when(me == 2)
    def _():
        pl.semaphore_wait(barrier, 2)
        for peer in (left, right):
            pl.semaphore_signal(ready, 1, device_id=(peer,), device_id_type=MESH)

    def first(buf, rows=slice(None), send=(None, None)):
        return [remote(buf.at[0, rows], buf.at[2, rows], right, send[0]),
                remote(buf.at[1, rows], buf.at[5, rows], left, send[1])]

    def second(buf, rows=slice(None), send=(None, None)):
        return [remote(buf.at[1, rows], buf.at[3, rows], right, send[0]),
                remote(buf.at[0, rows], buf.at[4, rows], left, send[1])]

    def forward(buf, rows=slice(None), send=(None, None)):
        return [remote(buf.at[2, rows], buf.at[6, rows], right, send[0]),
                remote(buf.at[5, rows], buf.at[7, rows], left, send[1])]

    def tile(n):
        return LOW_O + 32 * n

    rest = CUTS[-2] // 4
    early = [first(msg, slice(0, SUB))]
    early += [[remote(msg.at[0:2, a // 4:b // 4], msg.at[2:4, a // 4:b // 4], right),
               remote(msg.at[0:2, a // 4:b // 4], msg.at[4:6, a // 4:b // 4], left)]
              for a, b in pieces[1:-1]]
    early += [first(msg, slice(rest, PLANES_Q))]
    q1_planes = first(msg, slice(PLANES_Q, STREAM))
    q1_stream = first(msg, slice(STREAM, PLANES_O)) + first(top_q)
    q2 = second(msg, slice(rest, PLANES_O)) + second(top_q)
    o_tops = first(top_o) + second(top_o)
    qf_top, of_top = forward(top_q), forward(top_o)
    o1_a = first(msg, slice(PLANES_O, tile(3)), (2, 3))
    o1_b = first(msg, slice(tile(3), END), (2, 3))
    o2_a = second(msg, slice(PLANES_O, tile(1)), (2, 3))
    o2_b = second(msg, slice(tile(1), tile(3)), (2, 3))
    o2_c = second(msg, slice(tile(3), END), (2, 3))
    o_all = [remote(msg.at[0:2, PLANES_O:], msg.at[2:4, PLANES_O:], right, 2, 2),
             remote(msg.at[0:2, PLANES_O:], msg.at[4:6, PLANES_O:], left, 3, 3)]
    qf = forward(msg, slice(LOW_Q, PLANES_O), (4, 5))
    of_planes = forward(msg, slice(PLANES_O, LOW_O), (4, 5))
    of = [forward(msg, slice(tile(n), tile(n + 1)), (4, 5)) for n in range(4)]
    f_all = [remote(msg.at[2], msg.at[6], right, 4, 4), remote(msg.at[5], msg.at[7], left, 5, 5)]

    peak = [None, None]
    for n, (a, b) in enumerate(pieces):
        loaded(ld_wq[n])
        words = [to_words(wq32[a:b, h * LANES:(h + 1) * LANES]) for h in range(2)]
        for h in range(2):
            msg[h, a // 4:b // 4] = pack_low(words[h])
        pl.when(me >= 2)(early[n][0].start)
        pl.when((me == 1) | (me == 2))(early[n][1].start)
        for h in range(2):
            w[h, a // 2:b // 2] = words[h]
            peak[h] = running_max(words[h], peak[h])

    def encode(matrix, top):
        @pl.loop(0, 4)
        def _(i):
            h, j = i >> 1, 2 * matrix + (i & 1)
            rows = pl.ds(pl.multiple_of(j * 16 * SUB, 16 * SUB), 16 * SUB)
            parts[h, j] = cat(pack_high(vregs(w[h, rows]), top(h)))

    for h in range(2):
        top_q[h, 0] = column_max(peak[h])
    encode(0, lambda h: top_q[h, 0])
    for h in range(2):
        msg[h, PLANES_Q:STREAM] = cat(join_planes(vregs(parts[h, 0]), vregs(parts[h, 1])))

    @pl.when(me == 0)
    def _():
        pl.semaphore_wait(barrier, 2)

    @pl.when(odd)
    def _():
        pl.semaphore_wait(ready, 1)

    @pl.when(me < 2)
    def _():
        start([copies[0] for copies in early])

    @pl.when((me == 0) | (me == 3))
    def _():
        start([copies[1] for copies in early])

    start(q1_planes)
    pl.when(me != 3)(packed_head[0].start)
    pl.when(me != 1)(packed_head[1].start)

    for h in range(2):
        loaded(ld_wo[h])
        words = cat([to_words(wo32[h, :, n * LANES:(n + 1) * LANES]) for n in range(4)])
        w[h, WO:] = words
        msg[h, LOW_O:END] = pack_low(words)
        top_o[h] = column_max(running_max(words))
    encode(1, lambda h: top_o[h])
    for h in range(2):
        part = [vregs(parts[h, j]) for j in range(4)]
        bits, spare = join_runs([v[i:i + 2] for v in part for i in (4, 6)])
        msg[h, STREAM:LOW_O] = cat(bits + join_planes(part[2], part[3]))
        top_q[h, 1], top_q[h, 2] = spare
    start(q1_stream, q2, o1_a)

    stream, terms = {}, [0] * 4

    def gather(ref, slots, at):
        return cat([ref[g:g + 1, at] for g in slots])

    def decode_wq(*slots):
        spare = [jnp.where(upper_sublanes(), top_q[g, 2], top_q[g, 1])[None] for g in slots]
        bits = [gather(msg, slots, pl.ds(STREAM + i * SUB, SUB)) for i in range(2)] + [cat(spare)]
        high, stream[slots] = unpack_high(
            gather(msg, slots, slice(PLANES_Q, STREAM)), gather(top_q, slots, 0), bits)
        return [unpack_low(high[j], msg[g, LOW_Q:PLANES_Q], top_q[g, 0]) for j, g in enumerate(slots)]

    def decode_wo_high(*slots):
        high, _ = unpack_high(
            gather(msg, slots, slice(PLANES_O, LOW_O)), gather(top_o, slots, slice(None)), stream[slots])
        return [high[j] for j in range(len(slots))]

    def unpack_wq(*slots):
        for g, words in zip(slots, decode_wq(*slots)):
            w[g, :WO] = words

    def unpack_wo(*slots):
        for g, high in zip(slots, decode_wo_high(*slots)):
            w[g, WO:] = high

    def wo_tile(g, n):
        words = w[g, WO + BLK * n:WO + BLK * (n + 1)]
        if g >= 2:
            words = unpack_low(words, msg[g, tile(n):tile(n + 1)], top_o[g])
        return to_bf16(words)

    def differences(decoded, words):
        return functools.reduce(jnp.bitwise_or, vregs(decoded ^ words))

    def project_q(g, b=None, weights=w):
        rows = slice(None) if b is None else slice(b * S // 2, (b + 1) * S // 2)
        qbuf[g, rows] = to_words(jnp.dot(
            to_bf16(xb[rows]), to_bf16(weights[g, :WO]), preferred_element_type=F32))

    def keys(g):
        return [k32[g, b].astype(BF16).T for b in range(B)]

    def attend(g, p):
        for t in range(2):
            for b in range(B):
                ctx[g, (2 * b + t) * BLK:(2 * b + t + 1) * BLK] = context(*p[b], v32[g, b], t)

    def softmaxes(s):
        return [softmax(s[b]) for b in range(B)]

    def project_out(slots, *tiles):
        cols = slice(tiles[0] * LANES, (tiles[-1] + 1) * LANES)
        rhs = cat([jnp.concatenate([wo_tile(g, n) for n in tiles], 1) for g in slots])
        m = B * S * len(tiles) // 2
        for r in range(0, B * S, m):
            lhs = jnp.concatenate([to_bf16(ctx[g, r // 2:(r + m) // 2]) for g in slots], 1)
            res = jnp.dot(lhs, rhs, preferred_element_type=F32)
            if terms[tiles[0]] > 0:
                res = res + acc[r:r + m, cols]
            if terms[tiles[0]] == 3:
                out_ref[r:r + m, cols] = res.astype(out_ref.dtype)
            else:
                acc[r:r + m, cols] = res
        for n in tiles:
            terms[n] += 1

    loaded(ld_x[0])
    wrong = [differences(decoded, w[g, :WO]) for g, decoded in enumerate(decode_wq(0, 1))]
    xb[:S // 2] = to_words(x32[0] * SCALE)
    project_q(0, 0)
    project_q(1, 0)

    loaded(ld_x[1])
    for g, high in enumerate(decode_wo_high(0, 1)):
        decoded = unpack_low(high, msg[g, LOW_O:END], top_o[g])
        wrong[g] = differences(decoded, w[g, WO:]) | wrong[g]
        top_o[g] = top_o[g] | jnp.min(jnp.where(wrong[g] != 0, SIGN, 0), axis=0, keepdims=True)
    xb[S // 2:] = to_words(x32[1] * SCALE)
    project_q(0, 1)
    project_q(1, 1)

    loaded(ld_k[0], ld_k[1])
    s = [scores(qbuf[g], keys(g)) for g in range(2)]
    for g in range(2):
        for b, (e, inv) in enumerate(softmaxes(s[g])):
            pbuf[g, b] = cat(e + [jnp.broadcast_to(pltpu.bitcast(v, I32), (SUB, LANES)) for v in inv])

    loaded(ld_v[0], ld_v[1])
    start(o_tops)
    sent(*early, q1_planes)

    @pl.when(me == 0)
    def _():
        received(head)
        for j in range(2):
            msg[3 + j, 0:SUB] = pack_low(to_words(head32[j]))

    for j, sender in enumerate((3, 1)):
        pl.when(me == sender)(head[j].wait_send)
        pl.when(me != sender)(packed_head[j].wait_send)
        pl.when(me != 0)(packed_head[j].wait_recv)

    received(*early, q1_planes, q1_stream)
    start(qf_top, qf, o1_b, o2_a)
    unpack_wq(2, 5)
    for g in range(2):
        attend(g, [([pbuf[g, b, P_ROWS[i]:P_ROWS[i + 1]] for i in range(NB)],
                    [pltpu.bitcast(pbuf[g, b, pl.ds(P_ROWS[NB] + SUB * i, 1)], F32) for i in range(NB)])
                   for b in range(B)])
    project_q(2)
    project_q(5)
    project_out((0, 1), 0)

    loaded(ld_k[2], ld_k[5], ld_v[2], ld_v[5])
    received(q2)
    unpack_wq(3, 4)
    project_out((0, 1), 1)
    s = scores(qbuf[2], keys(2))
    project_q(3)
    attend(2, softmaxes(s))
    s = scores(qbuf[5], keys(5))
    project_q(4, 0)
    attend(5, softmaxes(s))
    project_q(4, 1)

    loaded(ld_k[3], ld_k[4], ld_v[3], ld_v[4])
    received(o1_a, o_tops)
    start(of_top, of_planes, o2_b, o2_c, *of[:3])
    unpack_wo(2, 5)
    project_out((0, 1), 2)
    s = [scores(qbuf[g], keys(g)) for g in (3, 4)]
    project_out((0, 1), 3)
    attend(3, softmaxes(s[0]))
    attend(4, softmaxes(s[1]))
    project_out((2, 5), 0)

    loaded(ld_k[6], ld_k[7], ld_v[6], ld_v[7])
    sent(q1_stream, q2, o_tops, qf_top)
    received(qf_top, qf)
    unpack_wq(6, 7)
    project_out((2, 5), 1, 2)
    project_q(6)
    project_q(7)
    for j in range(2):
        for b, k in enumerate(keys(6 + j)):
            kbuf[j, b] = pltpu.bitcast(k, I32)

    received(o1_b)
    start(of[3])
    received(o2_a)
    unpack_wo(3, 4)
    s = [scores(qbuf[6 + j], [to_bf16(kbuf[j, b]) for b in range(B)]) for j in range(2)]
    project_out((2, 5), 3)
    attend(6, softmaxes(s[0]))
    attend(7, softmaxes(s[1]))
    project_out((3, 4), 0)

    received(of_top, of_planes, o2_b)
    unpack_wo(6, 7)
    inexact = jnp.min(functools.reduce(jnp.bitwise_or, [top_o[g] for g in range(8)])) < 0
    project_out((3, 4), 1, 2)

    sent(of_top)
    received(o2_c, of[0])
    project_out((3, 4), 3)
    project_out((6, 7), 0)
    for n in (1, 2):
        received(of[n])
        project_out((6, 7), n)
    sent(o_all, f_all)
    received(of[3])
    project_out((6, 7), 3)

    @pl.when(inexact)
    def _():
        plain[0:2] = w[0:2]
        copies = [first(plain), second(plain), forward(plain)]
        start(*copies[:2])
        received(copies[0])
        start(copies[2])
        acc[...] = jnp.zeros(acc.shape, F32)
        received(*copies[1:])
        sent(*copies)

        @pl.loop(0, 8)
        def _(g):
            project_q(g, weights=plain)
            attend(g, softmaxes(scores(qbuf[g], keys(g))))
            for n in range(4):
                acc[:, n * LANES:(n + 1) * LANES] += jnp.dot(
                    to_bf16(ctx[g]), to_bf16(plain[g, WO + BLK * n:WO + BLK * (n + 1)]),
                    preferred_element_type=F32)

        out_ref[...] = acc[...].astype(out_ref.dtype)


def pallas_dist_sparse_attn_causalblk_htp_bs_b2_sq256_skv256_hq4_dh64_kernel(
    x: jax.Array,
    Wq: jax.Array,
    K_ext: jax.Array,
    V_ext: jax.Array,
    Wo: jax.Array,
):
    batch, seq, heads, dim = K_ext.shape
    kt = jnp.transpose(K_ext, (0, 2, 3, 1)).reshape(batch, heads * dim, seq)
    vt = jnp.transpose(V_ext, (0, 2, 3, 1)).reshape(batch, heads * dim, seq)
    out = pl.pallas_call(
        kernel_body,
        out_shape=jax.ShapeDtypeStruct((B * S, D), BF16),
        in_specs=[pl.BlockSpec(memory_space=pl.ANY)] * 5,
        out_specs=pl.BlockSpec(memory_space=pltpu.VMEM),
        scratch_shapes=[
            pltpu.VMEM((D, 2 * LANES), F32),
            pltpu.VMEM((2, LANES, D), F32),
            pltpu.VMEM((B, S, D), F32),
            pltpu.VMEM((8, B, LANES, S), F32),
            pltpu.VMEM((8, B, LANES, S), F32),
            pltpu.VMEM((2, CUTS[1], LANES), F32),
            pltpu.VMEM((8, D, LANES), I32),
            pltpu.VMEM((8, D, LANES), I32),
            pltpu.VMEM((8, END, LANES), I32),
            pltpu.VMEM((8, 3, 1, LANES), I32),
            pltpu.VMEM((8, 1, LANES), I32),
            pltpu.VMEM((2, 4, 8 * SUB, LANES), I32),
            pltpu.VMEM((B * S // 2, D), I32),
            pltpu.VMEM((8, B * S // 2, LANES), I32),
            pltpu.VMEM((2, B, S // 2, LANES), I32),
            pltpu.VMEM((2, B, P_ROWS[NB] + NB * SUB, LANES), I32),
            pltpu.VMEM((8, B * S // 2, LANES), I32),
            pltpu.VMEM((B * S, D), F32),
            pltpu.SemaphoreType.DMA((25,)),
            pltpu.SemaphoreType.DMA((62,)),
            pltpu.SemaphoreType.DMA((62,)),
            pltpu.SemaphoreType.REGULAR,
        ],
        compiler_params=pltpu.CompilerParams(
            collective_id=0,
            vmem_limit_bytes=48 * 1024 * 1024,
            disable_semaphore_checks=True,
            flags={"XLA_TPU_FORCE_LP_LLO_SCHEDULER": True},
        ),
    )(x, Wq, kt, vt, Wo)
    return out.reshape(x.shape)
```
